```python
import numpy as np

kernel_name = "dist_layernorm_xy_m512_n256"

def setup_inputs():
    x = np.random.randn(1024, 512).astype(np.float32)
    gamma = np.random.randn(512).astype(np.float32)
    beta = np.random.randn(512).astype(np.float32)
    return {"x": x, "gamma": gamma, "beta": beta}

def reference(x: np.ndarray, gamma: np.ndarray, beta: np.ndarray) -> np.ndarray:
    eps = 1e-5
    mean = np.mean(x, axis=1, keepdims=True)
    var = np.var(x, axis=1, keepdims=True)
    return gamma * (x - mean) / np.sqrt(var + eps) + beta
```

```python
import jax
import jax.numpy as jnp
from jax import lax
from jax.experimental import pallas as pl
from jax.experimental.pallas import tpu as pltpu

EPS = 1e-5
CHUNKS = (128, 128, 128, 128)


def pallas_dist_layernorm_xy_m512_n256_kernel(
    x: jax.Array,
    gamma: jax.Array,
    beta: jax.Array,
):
    m, n = x.shape
    nc = len(CHUNKS)
    starts = [sum(CHUNKS[:i]) for i in range(nc)]

    def body(x_hbm, g_hbm, b_hbm, o_ref, xv, gv, bv, st, rx, isem, psem, ssem, rsem):
        loads = []
        for i in range(nc):
            rows = pl.ds(starts[i], CHUNKS[i])
            c = pltpu.make_async_copy(x_hbm.at[rows], xv.at[rows], isem.at[i])
            c.start()
            loads.append(c)
        cg = pltpu.make_async_copy(g_hbm, gv, psem.at[0])
        cg.start()
        cb = pltpu.make_async_copy(b_hbm, bv, psem.at[1])
        cb.start()
        nbr = (lax.axis_index("x"), 1 - lax.axis_index("y"))
        bar = pltpu.get_barrier_semaphore()
        pl.semaphore_signal(bar, inc=1, device_id=nbr, device_id_type=pl.DeviceIdType.MESH)

        off = lax.broadcasted_iota(jnp.int32, (8, 128), 1) - lax.broadcasted_iota(jnp.int32, (8, 128), 0)
        rd = []
        for i in range(nc):
            loads[i].wait()
            acc_h = jnp.zeros((8, 128), jnp.float32)
            acc_v = jnp.zeros((8, 128), jnp.float32)
            for j in range(CHUNKS[i] // 8):
                r = pl.ds(starts[i] + 8 * j, 8)
                a, b = xv[r, 0:128], xv[r, 128:256]
                mu = jnp.sum((a + b) * (1.0 / n), axis=1, keepdims=True)
                da, db = a - mu, b - mu
                q = jnp.sum((da * da + db * db) * (0.5 / n), axis=1, keepdims=True)
                acc_h = jnp.where(off == 8 * j, mu, acc_h)
                acc_v = jnp.where(off == 8 * j, q, acc_v)
            st[i, 0:1, :] = jnp.sum(acc_h, axis=0, keepdims=True)
            st[i, 1:2, :] = jnp.sum(acc_v, axis=0, keepdims=True)
            if i == 0:
                pl.semaphore_wait(bar, 1)
            c = pltpu.make_async_remote_copy(
                st.at[i], rx.at[i], ssem.at[i], rsem.at[i],
                device_id=nbr, device_id_type=pl.DeviceIdType.MESH)
            c.start()
            rd.append(c)
        cg.wait()
        cb.wait()
        g = jnp.broadcast_to(gv[...], (8, n))
        be = jnp.broadcast_to(bv[...], (8, n))
        for i in range(nc):
            rd[i].wait_send()
        for i in range(nc):
            rd[i].wait_recv()
            ml = jnp.broadcast_to(st[i, 0:1, :], (8, 128))
            vl = jnp.broadcast_to(st[i, 1:2, :], (8, 128))
            mp = jnp.broadcast_to(rx[i, 0:1, :], (8, 128))
            vp = jnp.broadcast_to(rx[i, 1:2, :], (8, 128))
            mean = 0.5 * (ml + mp)
            dl = 0.5 * (ml - mp)
            rs = lax.rsqrt(dl * dl + (vl + EPS + vp))
            for j in range(CHUNKS[i] // 16):
                outs = []
                for k in (2 * j, 2 * j + 1):
                    r = pl.ds(starts[i] + 8 * k, 8)
                    mb = jnp.sum(jnp.where(off == 8 * k, mean, 0.0), axis=1, keepdims=True)
                    rb = jnp.sum(jnp.where(off == 8 * k, rs, 0.0), axis=1, keepdims=True)
                    outs.append((xv[r, :] - mb) * g * rb + be)
                o_ref[pl.ds(starts[i] + 16 * j, 16), :] = jnp.concatenate(outs, axis=0).astype(o_ref.dtype)

    return pl.pallas_call(
        body,
        out_shape=jax.ShapeDtypeStruct((m, n), jnp.bfloat16),
        in_specs=[pl.BlockSpec(memory_space=pltpu.HBM)] * 3,
        out_specs=pl.BlockSpec(memory_space=pltpu.VMEM),
        scratch_shapes=[
            pltpu.VMEM((m, n), jnp.float32),
            pltpu.VMEM((1, n), jnp.float32),
            pltpu.VMEM((1, n), jnp.float32),
            pltpu.VMEM((nc, 2, 128), jnp.float32),
            pltpu.VMEM((nc, 2, 128), jnp.float32),
            pltpu.SemaphoreType.DMA((nc,)),
            pltpu.SemaphoreType.DMA((2,)),
            pltpu.SemaphoreType.DMA((nc,)),
            pltpu.SemaphoreType.DMA((nc,)),
        ],
        compiler_params=pltpu.CompilerParams(
            collective_id=0, disable_bounds_checks=True, disable_semaphore_checks=True),
    )(x, gamma.reshape(1, n), beta.reshape(1, n))
```

```python
import jax
import jax.numpy as jnp
from jax import lax
from jax.experimental import pallas as pl
from jax.experimental.pallas import tpu as pltpu

EPS = 1e-5
SUBLANES, LANES = 8, 128

GROUPS = (15, 15, 10, 12, 6, 6)
SHIFT_MESSAGES = ((0, 1), (2,), (3, 4, 5))
PAIRED = (2, 3, 4)
LOAD_ORDER = (
    (0, 0), (1, 0), (0, 1), (2, 0), (1, 1), (3, 0),
    (2, 1), (4, 0), (5, 0), (3, 1), (4, 1), (5, 1),
)


def _pack(low, high):
    def bits(v):
        rounded = v.astype(jnp.bfloat16).astype(jnp.float32)
        return lax.bitcast_convert_type(rounded, jnp.int32)

    word = bits(high) | lax.shift_right_logical(bits(low), 16)
    return lax.bitcast_convert_type(word, jnp.float32)


def _unpack(packed):
    word = lax.bitcast_convert_type(packed, jnp.int32)
    low = lax.bitcast_convert_type(word << 16, jnp.float32)
    high = lax.bitcast_convert_type(word & -65536, jnp.float32)
    return low, high


def pallas_dist_layernorm_xy_m512_n256_kernel(
    x: jax.Array,
    gamma: jax.Array,
    beta: jax.Array,
):
    m, n = x.shape
    assert n == 2 * LANES and m == SUBLANES * sum(GROUPS)
    n_chunks, n_shift_msgs = len(GROUPS), len(SHIFT_MESSAGES)
    first = [sum(GROUPS[:c]) for c in range(n_chunks)]
    groups = [range(first[c], first[c] + GROUPS[c]) for c in range(n_chunks)]

    parked_chunks = (4, 3)
    shift_slot = n_chunks
    park_slot = shift_slot + n_shift_msgs
    term_slot = park_slot + len(parked_chunks)
    n_slots = term_slot + 3 * n_chunks

    def body(
        x_hbm, gamma_hbm, beta_hbm, out_ref,
        x_ref, inbox, own_ref, gamma_ref, beta_ref,
        load_sems, param_sems, send_sems, recv_sems, fence_sem,
        stats_out, shifts_out,
    ):
        loads = {}
        for c, half in LOAD_ORDER:
            block = (
                pl.ds(SUBLANES * first[c], SUBLANES * GROUPS[c]),
                pl.ds(LANES * half, LANES),
            )
            loads[c, half] = pltpu.make_async_copy(
                x_hbm.at[block], x_ref.at[block], load_sems.at[2 * c + half]
            )
            loads[c, half].start(priority=int(len(loads) > 1))
        gamma_load = pltpu.make_async_copy(gamma_hbm, gamma_ref, param_sems.at[0])
        gamma_load.start(priority=1)
        beta_load = pltpu.make_async_copy(beta_hbm, beta_ref, param_sems.at[1])
        beta_load.start(priority=1)

        peer = (lax.axis_index("x"), 1 - lax.axis_index("y"))
        barrier = pltpu.get_barrier_semaphore()
        pl.semaphore_signal(
            barrier, inc=1, device_id=peer, device_id_type=pl.DeviceIdType.MESH
        )
        for ref in (*stats_out, own_ref):
            ref[...] = jnp.zeros(ref.shape, ref.dtype)

        tile = (SUBLANES, LANES)
        diagonal = lax.broadcasted_iota(jnp.int32, tile, 1) - lax.broadcasted_iota(
            jnp.int32, tile, 0
        )
        left, right = pl.ds(0, LANES), pl.ds(LANES, LANES)

        def rows(g):
            return pl.ds(SUBLANES * g, SUBLANES)

        def side_rows(g):
            return pl.ds(m + SUBLANES * g, SUBLANES)

        def lane_sum(v):
            return jnp.broadcast_to(jnp.sum(v, axis=1, keepdims=True), tile)

        def read_row(ref, r):
            return jnp.broadcast_to(ref[r : r + 1, :], tile)

        def pick(v, i):
            return jnp.where(diagonal == SUBLANES * i, v, 0.0)

        def both_halves(v):
            return jnp.concatenate([v, v], axis=1)

        def fence():
            pl.semaphore_signal(fence_sem, 1)
            pl.semaphore_wait(fence_sem, 1)

        def to_peer(src, slot):
            return pltpu.make_async_remote_copy(
                src,
                inbox.at[pl.ds(SUBLANES * slot, src.shape[0])],
                send_sems.at[slot],
                recv_sems.at[slot],
                device_id=peer,
                device_id_type=pl.DeviceIdType.MESH,
            )

        stats_msgs = [to_peer(stats_out[c], c) for c in range(n_chunks)]
        shift_msgs = [to_peer(shifts_out[i], shift_slot + i) for i in range(n_shift_msgs)]

        shift, half_shift_row, sums, parked_shifts = {}, {}, {}, set()

        def find_shift(c):
            row = jnp.zeros(tile, jnp.float32)
            for i, g in enumerate(groups[c]):
                shift[g] = lane_sum(x_ref[rows(g), left] * (1.0 / LANES))
                row = jnp.where(diagonal == SUBLANES * i, shift[g], row)
            half_shift_row[c] = jnp.sum(row, axis=0, keepdims=True) * 0.5

        def park_shift(c):
            for g in groups[c]:
                x_ref[side_rows(g), left] = shift[g]
            parked_shifts.add(c)

        def shift_of(c, g):
            return x_ref[side_rows(g), left] if c in parked_shifts else shift[g]

        def reduce_rows(c, park=False):
            linear, square = [], []
            for g in groups[c]:
                k = shift_of(c, g)
                a, b = x_ref[rows(g), left] - k, x_ref[rows(g), right] - k
                linear.append(a + b)
                square.append(a * a + b * b)
            if park:
                x_ref[side_rows(first[c]), right] = square[0]
                square[0] = x_ref[side_rows(first[c]), right]
            scale = jnp.full(tile, 1.0 / (2 * n), jnp.float32)
            sums[c] = [
                lax.dot_general(
                    scale,
                    jnp.concatenate(terms, axis=0),
                    (((1,), (1,)), ((), ())),
                    preferred_element_type=jnp.float32,
                )
                for terms in (linear, square)
            ]

        def send_stats(c):
            s, q = sums[c]
            lanes = pl.ds(0, SUBLANES * GROUPS[c])
            stats_out[c][:, lanes] = _pack(s, q)[0:1]
            stats_msgs[c].start()
            own_ref[pl.ds(SUBLANES * c, 1), lanes] = s[0:1]
            own_ref[pl.ds(SUBLANES * c + 1, 1), lanes] = q[0:1]

        def send_shifts(i):
            for r, c in enumerate(SHIFT_MESSAGES[i]):
                shifts_out[i][r : r + 1, :] = half_shift_row[c]
            shift_msgs[i].start()

        pl.semaphore_wait(barrier, 1)
        loads[0, 0].wait()
        find_shift(0)
        loads[1, 0].wait()
        fence()
        find_shift(1)
        loads[0, 1].wait()
        reduce_rows(0)
        send_shifts(0)
        loads[2, 0].wait()
        loads[1, 1].wait()
        find_shift(2)
        reduce_rows(1)
        send_stats(0)
        loads[3, 0].wait()
        park_shift(2)
        find_shift(3)
        send_stats(1)
        loads[2, 1].wait()
        loads[4, 0].wait()
        reduce_rows(2)
        loads[5, 0].wait()
        find_shift(4)
        find_shift(5)
        send_shifts(1)
        park_shift(3)
        loads[3, 1].wait()
        reduce_rows(3, park=True)
        loads[4, 1].wait()
        reduce_rows(4)
        send_stats(2)
        send_shifts(2)
        loads[5, 1].wait()
        reduce_rows(5)
        send_stats(3)
        send_stats(4)
        send_stats(5)

        fence()
        gamma_load.wait()
        beta_load.wait()
        for c in PAIRED:
            for g in groups[c]:
                x_ref[rows(g), :] = x_ref[rows(g), :] - both_halves(shift_of(c, g))
        for msg in stats_msgs + shift_msgs:
            msg.wait_send()
        fence()

        scale = jnp.broadcast_to(gamma_ref[...], (SUBLANES, n))
        bias = jnp.broadcast_to(beta_ref[...], (SUBLANES, n))
        spread = {}

        def prepare(c):
            i = next(i for i, chunks in enumerate(SHIFT_MESSAGES) if c in chunks)
            r = SHIFT_MESSAGES[i].index(c)
            s, q = read_row(own_ref, SUBLANES * c), read_row(own_ref, SUBLANES * c + 1)
            k_own = read_row(shifts_out[i], r)
            k_peer = read_row(inbox, SUBLANES * (shift_slot + i) + r)
            e = (k_own - k_peer) + s
            centre = (s + s) - e if c in PAIRED else (k_own + k_peer) + s
            terms = (e + e, ((q - s * (s + s)) + EPS) + e * e, centre)
            for t, value in enumerate(terms):
                inbox[rows(term_slot + 3 * c + t), :] = value

        def combine(c):
            twice_e, base, centre = (
                inbox[rows(term_slot + 3 * c + t), :] for t in range(3)
            )
            s, q = _unpack(read_row(inbox, SUBLANES * c))
            centre = centre + s
            var = jnp.maximum((base + q) - s * (s + twice_e), EPS)
            inv_std = jnp.exp2(-0.5 * jnp.log2(var))
            last = _pack(centre, inv_std) if c in PAIRED else inv_std
            for i, g in enumerate(groups[c]):
                picked = pick(last, i)
                if c in parked_chunks and g == groups[c][-1]:
                    slot = rows(park_slot + parked_chunks.index(c))
                    inbox[slot, :] = picked
                    picked = inbox[slot, :]
                if c in PAIRED:
                    spread[g] = [lane_sum(picked)]
                else:
                    spread[g] = [lane_sum(pick(centre, i)), lane_sum(picked)]

        def normalise(c):
            for g in groups[c]:
                centre, inv_std = _unpack(*spread[g]) if c in PAIRED else spread[g]
                y = (x_ref[rows(g), :] - both_halves(centre)) * scale
                y = y * both_halves(inv_std) + bias
                out_ref[rows(g), :] = y.astype(out_ref.dtype)

        shift_msgs[0].wait_recv()
        prepare(1)
        prepare(0)
        stats_msgs[0].wait_recv()
        combine(0)
        normalise(0)
        stats_msgs[1].wait_recv()
        combine(1)
        shift_msgs[1].wait_recv()
        normalise(1)
        prepare(2)
        fence()
        stats_msgs[2].wait_recv()
        combine(2)
        shift_msgs[2].wait_recv()
        prepare(3)
        prepare(4)
        prepare(5)
        stats_msgs[3].wait_recv()
        normalise(2)
        combine(3)
        stats_msgs[4].wait_recv()
        combine(4)
        stats_msgs[5].wait_recv()
        combine(5)
        normalise(5)
        normalise(4)
        normalise(3)

    hbm = pl.BlockSpec(memory_space=pltpu.HBM)
    n_msgs = n_chunks + n_shift_msgs
    return pl.pallas_call(
        body,
        out_shape=jax.ShapeDtypeStruct((m, n), jnp.bfloat16),
        in_specs=[hbm, hbm, hbm],
        out_specs=pl.BlockSpec(memory_space=pltpu.VMEM),
        scratch_shapes=[
            pltpu.VMEM((2 * m, n), jnp.float32),
            pltpu.VMEM((SUBLANES * n_slots, LANES), jnp.float32),
            pltpu.VMEM((SUBLANES * n_chunks, LANES), jnp.float32),
            pltpu.VMEM((1, n), jnp.float32),
            pltpu.VMEM((1, n), jnp.float32),
            pltpu.SemaphoreType.DMA((2 * n_chunks,)),
            pltpu.SemaphoreType.DMA((2,)),
            pltpu.SemaphoreType.DMA((n_msgs,)),
            pltpu.SemaphoreType.DMA((n_msgs,)),
            pltpu.SemaphoreType.REGULAR,
            [pltpu.VMEM((1, LANES), jnp.float32) for _ in GROUPS],
            [pltpu.VMEM((len(c), LANES), jnp.float32) for c in SHIFT_MESSAGES],
        ],
        compiler_params=pltpu.CompilerParams(
            collective_id=0,
            disable_bounds_checks=True,
            disable_semaphore_checks=True,
            flags={
                "XLA_TPU_RESCHEDULE_DMA_DONES": True,
                "XLA_TPU_FORCE_LP_LLO_SCHEDULER": True,
            },
        ),
    )(x, gamma.reshape(1, n), beta.reshape(1, n))
```
